```python
import numpy as np

kernel_name = "dist_rope_attn_htp_bs_b2_sq512_d1024_hq8_dh128"

def setup_inputs():
    x = np.random.randn(8, 512, 1024).astype(np.float32)
    Wq = np.random.randn(1024, 4096).astype(np.float32) * 0.02
    Wk = np.random.randn(1024, 4096).astype(np.float32) * 0.02
    Wv = np.random.randn(1024, 4096).astype(np.float32) * 0.02
    Wo = np.random.randn(4096, 1024).astype(np.float32) * 0.02
    return {"x": x, "Wq": Wq, "Wk": Wk, "Wv": Wv, "Wo": Wo}

def reference(x, Wq, Wk, Wv, Wo):
    B, Sq, Hq, Dh = 8, 512, 32, 128
    inv = 1.0 / (10000.0 ** (np.arange(0, Dh, 2) / Dh))
    pos = np.arange(Sq)[:, None] * inv[None, :]
    cos = np.repeat(np.cos(pos), 2, axis=-1).astype(np.float32)
    sin = np.repeat(np.sin(pos), 2, axis=-1).astype(np.float32)
    def rot(t):
        t2 = t.reshape(B, Sq, Hq, Dh // 2, 2)
        t_r = np.stack([-t2[..., 1], t2[..., 0]], axis=-1).reshape(B, Sq, Hq, Dh)
        return t * cos[None, :, None, :] + t_r * sin[None, :, None, :]
    Q = rot((x @ Wq).reshape(B, Sq, Hq, Dh))
    K = rot((x @ Wk).reshape(B, Sq, Hq, Dh))
    V = (x @ Wv).reshape(B, Sq, Hq, Dh)
    s = np.einsum('bihd,bjhd->bhij', Q, K).astype(np.float32) * 0.08838834764831843
    s_max = s.max(axis=-1, keepdims=True)
    w = np.exp(s - s_max)
    w = w / w.sum(axis=-1, keepdims=True)
    ctx = np.einsum('bhij,bjhd->bihd', w, V).reshape(B, Sq, Hq * Dh)
    return ctx @ Wo
```

```python
import numpy as np
import jax
import jax.numpy as jnp
from jax import lax
from jax.experimental import pallas as pl
from jax.experimental.pallas import tpu as pltpu

S, D, H, DH = 512, 1024, 8, 128
NDEV = 4
BF = jnp.bfloat16
F32 = jnp.float32


def _tables():
    inv = 1.0 / (10000.0 ** (np.arange(0, DH, 2) / DH))
    pos = np.arange(S)[:, None] * inv[None, :]
    cos = np.repeat(np.cos(pos), 2, axis=-1)
    sin = np.repeat(np.sin(pos), 2, axis=-1)
    sign = np.where(np.arange(DH) % 2 == 0, -1.0, 1.0)[None, :]
    c = 0.08838834764831843 * np.log2(np.e)
    return np.stack([cos * c, sin * sign * c, cos, sin * sign]).astype(np.float32)


_TAB = _tables()


def pallas_dist_rope_attn_htp_bs_b2_sq512_d1024_hq8_dh128_kernel(x, Wq, Wk, Wv, Wo):
    def body(x_hbm, wq_hbm, wk_hbm, wv_hbm, wo_hbm, tab, out_hbm,
             xst, wst, wb, xbuf, q_s, k_s, v_s, c_s, sbuf, rbuf, acc0, ost,
             lsem, xs_sem, xr_sem, ps_sem, pr_sem, osem):
        me = lax.axis_index("i")
        left = (me + NDEV - 1) % NDEV
        right = (me + 1) % NDEV

        def rcopy(src, dst, ssem, rsem, dev):
            return pltpu.make_async_remote_copy(
                src_ref=src, dst_ref=dst, send_sem=ssem, recv_sem=rsem,
                device_id=(dev,), device_id_type=pl.DeviceIdType.MESH)

        def xsend(k, src, dst, dev):
            return rcopy(xbuf.at[src], xbuf.at[dst], xs_sem.at[k], xr_sem.at[dst], dev)

        x_sends = [(0, 1, right), (7, 4, left), (1, 2, right), (4, 3, left),
                   (7, 6, right), (0, 5, left)]

        xl = [pltpu.make_async_copy(x_hbm.at[b], xst.at[b], lsem.at[b]) for b in range(2)]
        wl = [pltpu.make_async_copy(w, wst.at[i], lsem.at[2 + i])
              for i, w in enumerate((wq_hbm, wk_hbm, wv_hbm, wo_hbm))]
        xl[0].start()
        xl[1].start()
        for w in wl:
            w.start()
        xl[0].wait()
        xbuf[0] = xst[0].astype(BF)
        xsend(0, *x_sends[0]).start()
        xl[1].wait()
        xbuf[7] = xst[1].astype(BF)
        xsend(1, *x_sends[1]).start()

        def psend(s, dst, dev):
            return rcopy(sbuf.at[s - 1], rbuf.at[dst], ps_sem.at[s - 1], pr_sem.at[dst], dev)

        p_sends = {1: (4, left), 2: (0, right), 3: (3, left), 4: (2, right),
                   5: (1, right), 6: (5, left)}

        def xwait(slot):
            rcopy(xbuf.at[slot], xbuf.at[slot], xs_sem.at[0], xr_sem.at[slot], me).wait_recv()

        def pwait(slot):
            rcopy(rbuf.at[slot], rbuf.at[slot], ps_sem.at[0], pr_sem.at[slot], me).wait_recv()

        even = (lax.broadcasted_iota(jnp.int32, (S, DH), 1) % 2) == 0

        def rope(t, c, s):
            r = jnp.where(even, pltpu.roll(t, DH - 1, 1), pltpu.roll(t, 1, 1))
            return t * c + r * s

        def step(s, carry):
            for st in range(1, 7):
                @pl.when(s == st)
                def _(st=st):
                    if st == 1:
                        xwait(1)
                        xsend(2, *x_sends[2]).start()
                        xwait(4)
                        xsend(3, *x_sends[3]).start()
                    elif st == 2:
                        xsend(4, *x_sends[4]).start()
                        xsend(5, *x_sends[5]).start()
                        xwait(2)
                    elif st != 4:
                        xwait(st)

            def getw(i):
                @pl.when(s == 0)
                def _():
                    wl[i].wait()
                    wb[i] = wst[i].astype(BF)

            xb = xbuf[s]
            for i, dst in enumerate((q_s, k_s, v_s)):
                getw(i)
                for c in range(4):
                    r = jnp.dot(xb, wb[i, :, c * 256:(c + 1) * 256], preferred_element_type=F32)
                    for j in range(2):
                        t = r[:, j * DH:(j + 1) * DH]
                        if i < 2:
                            t = rope(t, tab[2 * i], tab[2 * i + 1])
                        dst[2 * c + j] = t.astype(BF)

            def head(h, carry):
                sc = lax.dot_general(q_s[h], k_s[h], (((1,), (1,)), ((), ())),
                                     preferred_element_type=F32)
                m = jnp.max(sc, axis=1, keepdims=True)
                p = jnp.exp2(sc - m)
                l = jnp.sum(p, axis=1, keepdims=True)
                o = jnp.dot(p.astype(BF), v_s[h], preferred_element_type=F32)
                c_s[h] = (o * (1.0 / l)).astype(BF)
                return carry

            lax.fori_loop(0, H, head, 0, unroll=2)

            getw(3)
            ctx = jnp.concatenate([c_s[h] for h in range(H)], axis=1)
            part = jnp.dot(ctx, wb[3], preferred_element_type=F32)

            @pl.when(s == 0)
            def _():
                acc0[...] = part

            @pl.when(s == 7)
            def _():
                pwait(2)
                pwait(5)
                ost[1] = part + rbuf[2].astype(F32) + rbuf[5].astype(F32)
                pltpu.make_async_copy(ost.at[1], out_hbm.at[1], osem.at[1]).start()

            @pl.when(s == 5)
            def _():
                pwait(0)

            @pl.when(s == 6)
            def _():
                pwait(3)

            @pl.when((s == 5) | (s == 6))
            def _():
                sbuf[s - 1] = (part + rbuf[jnp.where(s == 5, 0, 3)].astype(F32)).astype(BF)

            @pl.when((s >= 1) & (s <= 4))
            def _():
                sbuf[s - 1] = part.astype(BF)

            for st in range(1, 7):
                @pl.when(s == st)
                def _(st=st):
                    psend(st, *p_sends[st]).start()
                    if st == 6:
                        pwait(1)
                        pwait(4)
                        ost[0] = acc0[...] + rbuf[1].astype(F32) + rbuf[4].astype(F32)
                        pltpu.make_async_copy(ost.at[0], out_hbm.at[0], osem.at[0]).start()
            return carry

        lax.fori_loop(0, 8, step, 0)

        for k in range(6):
            xsend(k, *x_sends[k]).wait_send()
        for st in range(1, 7):
            psend(st, *p_sends[st]).wait_send()
        for b in range(2):
            pltpu.make_async_copy(ost.at[b], out_hbm.at[b], osem.at[b]).wait()

    any_spec = pl.BlockSpec(memory_space=pl.ANY)
    return pl.pallas_call(
        body,
        out_shape=jax.ShapeDtypeStruct((2, S, D), F32),
        in_specs=[any_spec] * 5 + [pl.BlockSpec(memory_space=pltpu.VMEM)],
        out_specs=any_spec,
        scratch_shapes=[
            pltpu.VMEM((2, S, D), F32),
            pltpu.VMEM((4, D, D), F32),
            pltpu.VMEM((4, D, D), BF),
            pltpu.VMEM((8, S, D), BF),
            pltpu.VMEM((H, S, DH), BF),
            pltpu.VMEM((H, S, DH), BF),
            pltpu.VMEM((H, S, DH), BF),
            pltpu.VMEM((H, S, DH), BF),
            pltpu.VMEM((6, S, D), BF),
            pltpu.VMEM((6, S, D), BF),
            pltpu.VMEM((S, D), F32),
            pltpu.VMEM((2, S, D), F32),
            pltpu.SemaphoreType.DMA((6,)),
            pltpu.SemaphoreType.DMA((6,)),
            pltpu.SemaphoreType.DMA((8,)),
            pltpu.SemaphoreType.DMA((6,)),
            pltpu.SemaphoreType.DMA((6,)),
            pltpu.SemaphoreType.DMA((2,)),
        ],
        compiler_params=pltpu.CompilerParams(vmem_limit_bytes=100 * 1024 * 1024),
    )(x, Wq, Wk, Wv, Wo, jnp.asarray(_TAB))
```

```python
import numpy as np
import jax
import jax.numpy as jnp
from jax import lax
from jax.experimental import pallas as pl
from jax.experimental.pallas import tpu as pltpu

S, D, H, DH = 512, 1024, 8, 128
NDEV = 4
BF = jnp.bfloat16
F32 = jnp.float32


def _tables():
    inv = 1.0 / (10000.0 ** (np.arange(0, DH, 2) / DH))
    pos = np.arange(S)[:, None] * inv[None, :]
    cos = np.repeat(np.cos(pos), 2, axis=-1)
    sin = np.repeat(np.sin(pos), 2, axis=-1)
    sign = np.where(np.arange(DH) % 2 == 0, -1.0, 1.0)[None, :]
    c = 0.08838834764831843 * np.log2(np.e)
    return np.stack([cos * c, sin * sign * c, cos, sin * sign]).astype(np.float32)


_TAB = _tables()


def pallas_dist_rope_attn_htp_bs_b2_sq512_d1024_hq8_dh128_kernel(x, Wq, Wk, Wv, Wo):
    def body(x_hbm, wq_hbm, wk_hbm, wv_hbm, wo_hbm, tab, out_hbm,
             xst, wst, wb, xbuf, sbuf, rbuf, acc0, ost,
             lsem, xs_sem, xr_sem, ps_sem, pr_sem, osem):
        me = lax.axis_index("i")
        left = (me + NDEV - 1) % NDEV
        right = (me + 1) % NDEV

        def rcopy(src, dst, ssem, rsem, dev):
            return pltpu.make_async_remote_copy(
                src_ref=src, dst_ref=dst, send_sem=ssem, recv_sem=rsem,
                device_id=(dev,), device_id_type=pl.DeviceIdType.MESH)

        def xsend(k, src, dst, dev):
            return rcopy(xbuf.at[src], xbuf.at[dst], xs_sem.at[k], xr_sem.at[dst], dev)

        x_sends = [(0, 1, right), (7, 4, left), (1, 2, right), (4, 3, left),
                   (7, 6, right), (0, 5, left)]

        xl = [pltpu.make_async_copy(x_hbm.at[b], xst.at[b], lsem.at[b]) for b in range(2)]
        ws = (wq_hbm, wk_hbm, wv_hbm)
        order = [(i, c) for c in range(4) for i in range(3)] + [(3, c) for c in range(4)]

        def wcopy(n):
            i, c = order[n]
            cs = pl.ds(c * 256, 256)
            if i < 3:
                return pltpu.make_async_copy(ws[i].at[:, cs], wst.at[i, :, cs], lsem.at[2 + n])
            return pltpu.make_async_copy(wo_hbm.at[cs, :], wst.at[3, cs, :], lsem.at[2 + n])

        AHEAD = 3
        xl[0].start()
        wcopy(0).start()
        bar = pltpu.get_barrier_semaphore()
        for nb in (left, right):
            pl.semaphore_signal(bar, inc=1, device_id=(nb,), device_id_type=pl.DeviceIdType.MESH)
        xl[0].wait()
        for n in range(1, AHEAD):
            wcopy(n).start()
        xbuf[0] = xst[0].astype(BF)
        pl.semaphore_wait(bar, 2)
        xsend(0, *x_sends[0]).start()

        def getw(n):
            i, c = order[n]
            wcopy(n).wait()
            if n == 0:
                xl[1].start()
            if n + AHEAD < len(order):
                wcopy(n + AHEAD).start()
            cs = pl.ds(c * 256, 256)
            if i < 3:
                wb[i, :, cs] = wst[i, :, cs].astype(BF)
            else:
                wb[3, cs, :] = wst[3, cs, :].astype(BF)

        def psend(s, dst, dev):
            return rcopy(sbuf.at[s - 1], rbuf.at[dst], ps_sem.at[s - 1], pr_sem.at[dst], dev)

        p_sends = {1: (4, left), 2: (0, right), 3: (3, left), 4: (2, right),
                   5: (1, right), 6: (5, left)}

        def xwait(slot):
            rcopy(xbuf.at[slot], xbuf.at[slot], xs_sem.at[0], xr_sem.at[slot], me).wait_recv()

        def pwait(slot):
            rcopy(rbuf.at[slot], rbuf.at[slot], ps_sem.at[0], pr_sem.at[slot], me).wait_recv()

        even = (lax.broadcasted_iota(jnp.int32, (S, DH), 1) % 2) == 0

        def rope(t, c, s):
            r = jnp.where(even, pltpu.roll(t, DH - 1, 1), pltpu.roll(t, 1, 1))
            return t * c + r * s

        def compute(xb, first, mid=None):
            outs = []
            for c in range(4):
                qkv = []
                for i in range(3):
                    if first:
                        getw(3 * c + i)
                    r = jnp.dot(xb, wb[i, :, c * 256:(c + 1) * 256], preferred_element_type=F32)
                    hs = []
                    for j in range(2):
                        t = r[:, j * DH:(j + 1) * DH]
                        if i < 2:
                            t = rope(t, tab[2 * i], tab[2 * i + 1])
                        hs.append(t.astype(BF))
                    qkv.append(hs)
                if first and c == 0:
                    xl[1].wait()
                    xbuf[7] = xst[1].astype(BF)
                    xsend(1, *x_sends[1]).start()
                for j in range(2):
                    sc = lax.dot_general(qkv[0][j], qkv[1][j], (((1,), (1,)), ((), ())),
                                         preferred_element_type=F32)
                    m = jnp.max(sc, axis=1, keepdims=True)
                    p = jnp.exp2(sc - m)
                    l = jnp.sum(p, axis=1, keepdims=True)
                    o = jnp.dot(p.astype(BF), qkv[2][j], preferred_element_type=F32)
                    outs.append((o * (1.0 / l)).astype(BF))
            if first:
                for n in range(12, 16):
                    getw(n)
            ctx = jnp.concatenate(outs, axis=1)
            return jnp.dot(ctx, wb[3], preferred_element_type=F32)

        acc0[...] = compute(xbuf[0], True)

        def step(s, carry):
            for st in range(1, 7):
                if st == 4:
                    continue

                @pl.when(s == st)
                def _(st=st):
                    if st == 1:
                        xwait(1)
                        xsend(2, *x_sends[2]).start()
                        xwait(4)
                        xsend(3, *x_sends[3]).start()
                    else:
                        if st == 2:
                            xsend(4, *x_sends[4]).start()
                        if st == 3:
                            xsend(5, *x_sends[5]).start()
                        xwait(st)

            part = compute(xbuf[s], False)

            @pl.when(s == 7)
            def _():
                pwait(2)
                pwait(5)
                ost[1] = part + rbuf[2].astype(F32) + rbuf[5].astype(F32)
                pltpu.make_async_copy(ost.at[1], out_hbm.at[1], osem.at[1]).start()

            @pl.when(s == 5)
            def _():
                pwait(0)

            @pl.when(s == 6)
            def _():
                pwait(3)

            @pl.when((s == 5) | (s == 6))
            def _():
                sbuf[s - 1] = (part + rbuf[jnp.where(s == 5, 0, 3)].astype(F32)).astype(BF)

            @pl.when(s <= 4)
            def _():
                sbuf[s - 1] = part.astype(BF)

            for st in range(1, 7):
                @pl.when(s == st)
                def _(st=st):
                    psend(st, *p_sends[st]).start()
                    if st == 6:
                        pwait(1)
                        pwait(4)
                        ost[0] = acc0[...] + rbuf[1].astype(F32) + rbuf[4].astype(F32)
                        pltpu.make_async_copy(ost.at[0], out_hbm.at[0], osem.at[0]).start()
            return carry

        lax.fori_loop(1, 8, step, 0)

        for k in range(6):
            xsend(k, *x_sends[k]).wait_send()
        for st in range(1, 7):
            psend(st, *p_sends[st]).wait_send()
        for b in range(2):
            pltpu.make_async_copy(ost.at[b], out_hbm.at[b], osem.at[b]).wait()

    any_spec = pl.BlockSpec(memory_space=pltpu.HBM)
    return pl.pallas_call(
        body,
        out_shape=jax.ShapeDtypeStruct((2, S, D), F32),
        in_specs=[any_spec] * 5 + [pl.BlockSpec(memory_space=pltpu.VMEM)],
        out_specs=any_spec,
        scratch_shapes=[
            pltpu.VMEM((2, S, D), F32),
            pltpu.VMEM((4, D, D), F32),
            pltpu.VMEM((4, D, D), BF),
            pltpu.VMEM((8, S, D), BF),
            pltpu.VMEM((6, S, D), BF),
            pltpu.VMEM((6, S, D), BF),
            pltpu.VMEM((S, D), F32),
            pltpu.VMEM((2, S, D), F32),
            pltpu.SemaphoreType.DMA((18,)),
            pltpu.SemaphoreType.DMA((6,)),
            pltpu.SemaphoreType.DMA((8,)),
            pltpu.SemaphoreType.DMA((6,)),
            pltpu.SemaphoreType.DMA((6,)),
            pltpu.SemaphoreType.DMA((2,)),
        ],
        compiler_params=pltpu.CompilerParams(collective_id=0, vmem_limit_bytes=100 * 1024 * 1024),
    )(x, Wq, Wk, Wv, Wo, jnp.asarray(_TAB))
```
